```python
import numpy as np

kernel_name = "dist_ar_xy_y_m1024_n512"

def setup_inputs():
    return {"x": np.random.randn(2048, 512).astype(np.float32)}

def reference(x: np.ndarray) -> np.ndarray:
    return x.reshape(2, 1024, 512).sum(axis=0)
```

```python
import jax
import jax.numpy as jnp
from jax import lax
from jax.experimental import pallas as pl
from jax.experimental.pallas import tpu as pltpu

MESH = pl.DeviceIdType.MESH
M, N = 1024, 512
H = M // 2
R = 16
K = 3
LOADS = (16, 48, 192, 256)
NC = H // R


def pallas_dist_ar_xy_y_m1024_n512_kernel(x: jax.Array):
    def body(x_hbm, o_ref, xv, sb, rb, ld_sem, ld2_sem, send_sem, ry, rx, xrdy):
        mx = lax.axis_index("x")
        my = lax.axis_index("y")
        ynbr = (mx, 1 - my)
        xnbr = (1 - mx, my)
        mine = pl.multiple_of(mx * H, H)
        lds = []
        off = 0
        for i, n in enumerate(LOADS):
            cp = pltpu.make_async_copy(x_hbm.at[pl.ds(mine + off, n)], xv.at[pl.ds(off, n)], ld_sem.at[i])
            cp.start()
            lds.append((off, n, cp))
            off += n
        bar = pltpu.get_barrier_semaphore()
        pl.semaphore_signal(bar, inc=1, device_id=ynbr, device_id_type=MESH)
        ex = pltpu.make_async_copy(x_hbm.at[pl.ds(M - K * R, K * R)], xv.at[pl.ds(H, K * R)], ld2_sem)

        @pl.when(mx == 0)
        def _():
            pl.semaphore_signal(bar, inc=1, device_id=xnbr, device_id_type=MESH)
            ex.start()

        def ycopy(c):
            return pltpu.make_async_remote_copy(
                sb.at[pl.ds(c * R, R)], rb.at[pl.ds(c * R, R)], send_sem.at[0], ry.at[c],
                device_id=ynbr, device_id_type=MESH)

        def xcopy(c):
            rows = o_ref.at[pl.ds(mine + c * R, R)]
            return pltpu.make_async_remote_copy(
                rows, rows, send_sem.at[1], rx.at[0], device_id=xnbr, device_id_type=MESH)

        for off, n, cp in lds:
            cp.wait()
            for c in range(off // R, (off + n) // R):
                sb[pl.ds(c * R, R), :] = xv[pl.ds(c * R, R), :].astype(jnp.bfloat16)
                if c == 0:
                    pl.semaphore_wait(bar, 1 + mx)
                ycopy(c).start()
                if c == 0:
                    @pl.when(mx == 1)
                    def _():
                        pl.semaphore_signal(xrdy, inc=1, device_id=xnbr, device_id_type=MESH)

        @pl.when(mx == 0)
        def _():
            ex.wait()
            for c in range(NC, NC + K):
                sb[pl.ds(c * R, R), :] = xv[pl.ds(c * R, R), :].astype(jnp.bfloat16)
                ycopy(c).start()

        def add(c):
            return (xv[pl.ds(c * R, R), :] + rb[pl.ds(c * R, R), :].astype(jnp.float32)).astype(jnp.bfloat16)

        for c in range(NC):
            ycopy(c).wait_recv()
            o_ref[pl.ds(mine + c * R, R), :] = add(c)
            if c == 0:
                @pl.when(mx == 0)
                def _():
                    pl.semaphore_wait(xrdy, 1)
            if c < NC - K:
                xcopy(c).start()
            else:
                @pl.when(mx == 0)
                def _():
                    xcopy(c).start()

        def wait_rows(n, sem):
            pltpu.make_async_copy(sb.at[pl.ds(0, n)], rb.at[pl.ds(0, n)], sem).wait()

        @pl.when(mx == 0)
        def _():
            for c in range(NC, NC + K):
                ycopy(c).wait_recv()
                o_ref[pl.ds(M - K * R + (c - NC) * R, R), :] = add(c)
            wait_rows(H + K * R, send_sem.at[0])
            wait_rows(H, send_sem.at[1])
            wait_rows(H - K * R, rx.at[0])

        @pl.when(mx == 1)
        def _():
            wait_rows(H, send_sem.at[0])
            wait_rows(H - K * R, send_sem.at[1])
            wait_rows(H, rx.at[0])

    return pl.pallas_call(
        body,
        out_shape=jax.ShapeDtypeStruct((M, N), jnp.bfloat16),
        in_specs=[pl.BlockSpec(memory_space=pltpu.HBM)],
        out_specs=pl.BlockSpec(memory_space=pltpu.VMEM),
        scratch_shapes=[
            pltpu.VMEM((H + K * R, N), jnp.float32),
            pltpu.VMEM((H + K * R, N), jnp.bfloat16),
            pltpu.VMEM((H + K * R, N), jnp.bfloat16),
            pltpu.SemaphoreType.DMA((len(LOADS),)),
            pltpu.SemaphoreType.DMA,
            pltpu.SemaphoreType.DMA((2,)),
            pltpu.SemaphoreType.DMA((NC + K,)),
            pltpu.SemaphoreType.DMA((1,)),
            pltpu.SemaphoreType.REGULAR,
        ],
        compiler_params=pltpu.CompilerParams(
            collective_id=0, disable_bounds_checks=True, disable_semaphore_checks=True),
    )(x)
```

```python
import jax
import jax.numpy as jnp
import numpy as np
from jax import lax
from jax.experimental import pallas as pl
from jax.experimental.pallas import tpu as pltpu

M, N = 1024, 512
HALF = M // 2
UNITS = HALF // 8

WORDS = 16
FULL = 14
POOL = 7
EARLY = 24
SIGNS = EARLY
HEADER = SIGNS + UNITS // 8
CODES = HEADER + 1
LATE = CODES + FULL
WIRE = LATE + UNITS - EARLY
EXTRA = 10
SPLIT = WIRE - EXTRA
RAW = WIRE + EXTRA
RAW_PARTS = [(RAW + i, min(8, UNITS - FULL - i)) for i in range(0, UNITS - FULL, 8)]

LOADS = (1, 1, 2) + (4,) * 15
GREET = 36
FIRST_FORWARDS = (56, 60)
LEAD = 28
OTHER_AT = 66
SLOT = 104
GROUP_ENDS = (LATE, 59, 67, 71, 74, 76, SPLIT, SPLIT + 4, SPLIT + 7, SPLIT + 9, WIRE)
GROUPS = [(a, b - a) for a, b in zip((0,) + GROUP_ENDS, GROUP_ENDS)]


def _i32(bits):
    return np.uint32(bits).astype(np.int32)


def _bytes(b):
    return _i32(b * 0x01010101)


EVEN, ODD, SIGN = _i32(0x00FF00FF), _i32(0xFF00FF00), _i32(0x80008000)
BORROW = _i32(0x01000100)


def _shl(a, n):
    return lax.shift_left(a, jnp.broadcast_to(n, a.shape))


def _shr(a, n):
    return lax.shift_right_logical(a, jnp.broadcast_to(n, a.shape))


def _wire(j):
    return j if j < EARLY else j - EARLY + LATE


def _live(j):
    n = 4 * (j + 1)
    return min(j + 1, WORDS, int(np.ceil((1.68 * n + 5.6 * np.sqrt(n) + 9) / 32)))


def _to_pairs(rows):
    tiles = [rows[:, c : c + 128] for c in range(0, N, 128)]
    return tuple(
        pltpu.bitcast(jnp.concatenate(tiles[i : i + 2], axis=0).astype(jnp.bfloat16), jnp.int32)
        for i in (0, 2)
    )


def _from_pairs(u, v):
    u, v = (pltpu.bitcast(w, jnp.bfloat16).astype(jnp.float32) for w in (u, v))
    return jnp.concatenate([u[:8], u[8:], v[:8], v[8:]], axis=1)


def _low_bytes(u, v):
    return (u & EVEN) | _shl(v & EVEN, 8)


def _high_bytes(u, v):
    return (_shr(u, 8) & EVEN) | (v & ODD)


def _reference(pairs):
    total = sum((w & 0x7FFF) + (_shr(w, 16) & 0x7FFF) for w in pairs).astype(jnp.float32)
    total = jnp.sum(jnp.sum(total, axis=1, keepdims=True), axis=0, keepdims=True)
    mean = jnp.broadcast_to(total, (8, 128)) * (1.0 / (2048 * len(pairs)))
    return jnp.minimum(mean.astype(jnp.int32) + 516, 0x7FFF)


def _sublane():
    return lax.broadcasted_iota(jnp.int32, (8, 128), 0)


def _or_sublanes(a):
    for shift in (4, 2, 1):
        a = a | pltpu.roll(a, shift, 0)
    return a


def _pool_rows(wanted):
    one = jnp.ones_like(wanted)
    return [
        lax.population_count(wanted & (_shl(one, _sublane() + 8 * i) - 1)) + 1
        for i in range(WORDS - FULL)
    ]


class _Encoder:
    def __init__(self, k):
        self.k = k
        self.k2 = k | _shl(k, 16) | SIGN
        zero = jnp.zeros_like(k)
        self.words = None
        self.bits, self.room, self.long, self.below_k = zero, zero, zero, ~zero

    def push(self, j, u, v):
        su, sv = u & SIGN, v & SIGN
        d = _high_bytes(self.k2 - (u ^ su), self.k2 - (v ^ sv))
        ge1, ge4 = (d - _bytes(1)) & _bytes(0x80), (d - _bytes(4)) & _bytes(0x80)
        size = (d - _bytes(0x7C)) + _shr(ge4, 7) - _shr(ge1, 5)
        end = size + _shl(size, 8)
        end = end + _shl(end, 16)
        one = jnp.ones_like(end)
        code = (one | _shl(one, end & 31)) | (
            _shl(one, _shr(end, 8) & 31) | _shl(one, _shr(end, 16) & 31)
        )
        self.below_k &= d
        self.long |= size | end
        self.bits += _shr(end, 24)
        if j == UNITS - 1 or _live(j + 1) != _live(j):
            self.room |= 32 * _live(j) - self.bits
        n = _shr(end, 24) & 31
        if j == 0:
            self.words = _shl(code, -n & 31)[None]
        else:
            old, kept = self.words, _shr(self.words, n)
            if _live(j) > old.shape[0]:
                kept = jnp.concatenate([kept, jnp.zeros_like(code)[None]])
            self.words = kept | _shl(jnp.concatenate([code[None], old])[: _live(j)], -n & 31)
        return _shr(su, 2 * (j % 8)) | _shr(sv, 2 * (j % 8) + 1)

    def header(self):
        misfit = (self.long & _bytes(0xE0)) | (~self.below_k & _bytes(0x80))
        misfit = jnp.where((misfit != 0) | (self.room < 0), 1, 0)
        fills = [self.bits > 32 * i for i in range(FULL, WORDS)]
        one = jnp.ones_like(misfit)
        wanted = sum(
            jnp.where(f, _shl(one, _sublane() + 8 * i), 0) for i, f in enumerate(fills)
        )
        wanted = _or_sublanes(wanted)
        misfit = _or_sublanes(misfit) | jnp.where(lax.population_count(wanted) > POOL, 1, 0)
        head = self.k | _shl(misfit, 15) | _shl(wanted, 16)
        rows = _pool_rows(wanted)
        for row in range(1, POOL + 1):
            word = sum(
                jnp.where(f & (r == row), self.words[FULL + i], 0)
                for i, (f, r) in enumerate(zip(fills, rows))
            )
            head = jnp.where(_sublane() == row, _or_sublanes(word), head)
        return head


class _Decoder:
    def __init__(self, wire, uncoded):
        self.wire = wire

        def row(i):
            return jnp.broadcast_to(wire[HEADER, pl.ds(i, 1), :], (8, 128))

        head = row(0)
        rows = _pool_rows(_shr(head, 16))
        pooled = [head] * len(rows)
        for i in range(1, POOL + 1):
            word = row(i)
            pooled = [jnp.where(r == i, word, w) for r, w in zip(rows, pooled)]
        words = jnp.concatenate([wire[pl.ds(CODES, FULL)]] + [w[None] for w in pooled])
        self.words = jnp.where(uncoded, -1, words)
        k = jnp.where(uncoded, 0xFF, head & 0x7FFF)
        high, low = _shl(_shr(k, 8) - 1, 8), (k & 0xFF) | 0x100
        self.k_high, self.k_low = high + _shl(high, 16), low | _shl(low, 16)
        self.left = UNITS
        self._scan()

    def _scan(self):
        word = self.words[0]
        self.zeros = [lax.clz(word)]
        for _ in range(3):
            word = _shl(_shl(word, 1), self.zeros[-1])
            self.zeros.append(lax.clz(word))

    def pop(self):
        j = self.left = self.left - 1
        z3, z2, z1, z0 = self.zeros
        if j:
            n = (z3 + 4) + z2 + z1
            n, rest = n + z0, (32 - n) - z0
            old, keep = self.words, _live(j - 1)
            self.words = _shl(old[:keep], n)
            if old.shape[0] > keep:
                self.words |= _shr(old[1 : keep + 1], rest)
            else:
                below = _shr(old[1:], rest)
                self.words |= jnp.concatenate([below, jnp.zeros_like(n)[None]])
            self._scan()
        rank = (z0 | _shl(z1, 8)) | (_shl(z2, 16) | _shl(z3, 24))
        ge3, ge4 = (rank + _bytes(0x7D)) & _bytes(0x80), (rank + _bytes(0x7C)) & _bytes(0x80)
        d = (rank + _bytes(1)) - _shr(ge3 ^ ge4, 5) - _shr(ge4, 7)
        signs = self.wire[SIGNS + j // 8]
        return (
            j,
            self.k_high - _shl(d & EVEN, 8) + (_shl(signs, 2 * (j % 8)) & SIGN),
            self.k_high - (d & ODD) + (_shl(signs, 2 * (j % 8) + 1) & SIGN),
        )

    def join(self, hu, hv, low):
        lu, lv = low & EVEN, _shr(low, 8) & EVEN
        return (
            hu + lu + ((self.k_low - lu) & BORROW),
            hv + lv + ((self.k_low - lv) & BORROW),
        )


def _kernel(
    x_hbm, out_ref, x_ref, tx, from_y, from_x, high_y, high_x,
    load_sems, y_sent, x_sent, y_sems, x_sems, raw_sems, x_started,
):
    my_x, my_y = lax.axis_index("x"), lax.axis_index("y")
    y_peer, x_peer = (my_x, 1 - my_y), (1 - my_x, my_y)
    mine, other = my_x * HALF, (1 - my_x) * HALF

    def rows(start, size=8):
        return pl.ds(start if isinstance(start, int) else pl.multiple_of(start, 8), size)

    def remote(src, dst, send_sem, recv_sem, peer):
        return pltpu.make_async_remote_copy(
            src, dst, send_sem, recv_sem, device_id=peer, device_id_type=pl.DeviceIdType.MESH
        )

    def signal(sem, peer):
        pl.semaphore_signal(sem, inc=1, device_id=peer, device_id_type=pl.DeviceIdType.MESH)

    def y_copy(p):
        return remote(tx.at[p], from_y.at[p], y_sent, y_sems.at[p], y_peer)

    def x_copy(p):
        group = sum(p >= end for end in GROUP_ENDS)
        return remote(from_y.at[p], from_x.at[p], x_sent, x_sems.at[group], x_peer)

    def raw_copy(i, hop):
        part, sem = pl.ds(*RAW_PARTS[i]), 2 * (hop * len(RAW_PARTS) + i)
        src, dst, peer = ((tx, from_y, y_peer), (from_y, from_x, x_peer))[hop]
        return remote(src.at[part], dst.at[part], raw_sems.at[sem], raw_sems.at[sem + 1], peer)

    def raw_at(j):
        return jnp.where(j < FULL, CODES + j, RAW + j - FULL)

    def misfits(wire):
        bit = wire[HEADER, pl.ds(0, 1), :] & 0x8000
        return jnp.max(bit.astype(jnp.float32), axis=1, keepdims=True)

    barrier = pltpu.get_barrier_semaphore()
    loads, first = {}, 0
    for i, n in enumerate(LOADS):
        loads[first] = pltpu.make_async_copy(
            x_hbm.at[rows(mine + 8 * first, 8 * n)], x_ref.at[rows(8 * first, 8 * n)], load_sems.at[i]
        )
        loads[first].start()
        first += n
        if i == 0:
            signal(barrier, y_peer)
            pl.when(my_x == 0)(lambda: signal(barrier, x_peer))
    load_other = pltpu.make_async_copy(
        x_hbm.at[rows(other, HALF)], x_ref.at[rows(HALF, HALF)], load_sems.at[len(LOADS)]
    )
    load_other.start()

    def greet():
        pl.semaphore_wait(barrier, 1 + my_x)
        y_copy(0).start()
        pl.when(my_x == 1)(lambda: signal(x_started, x_peer))

    def forward(p):
        y_copy(p).wait_recv()
        if p == 0:
            pl.when(my_x == 0)(lambda: pl.semaphore_wait(x_started, 1))
        if p < SPLIT:
            x_copy(p).start()
        else:
            pl.when(my_x == 0)(lambda: x_copy(p).start())

    sent = arrived = 0
    todo = []
    for j in range(UNITS):
        if j in loads:
            loads[j].wait()
        u, v = _to_pairs(x_ref[rows(8 * j), :])
        tx[_wire(j)] = _low_bytes(u, v)
        if j < EARLY:
            pl.when(my_y == 1)(greet if j == 0 else lambda: y_copy(j).start())
            sent += 1
        if j == GREET - 1:

            @pl.when(my_y == 0)
            def _():
                greet()
                for p in range(1, sent):
                    y_copy(p).start()

        todo.append((j, u, v))
        if j == 1:
            encoder = _Encoder(_reference([w for _, *pair in todo for w in pair]))
        while j >= 1 and todo:
            i, u, v = todo.pop(0)
            placed = encoder.push(i, u, v)
            signs = signs | placed if i % 8 else placed
            if i % 8 == 7:
                tx[SIGNS + i // 8] = signs
        while j >= GREET and sent < SIGNS + (j + 1) // 8:
            y_copy(sent).start()
            sent += 1
        if j in FIRST_FORWARDS:
            forward(arrived)
            arrived += 1
    tx[pl.ds(CODES, FULL)] = encoder.words[:FULL]
    forward(arrived)
    tx[HEADER] = encoder.header()
    forward(arrived + 1)
    found = misfits(tx)
    forward(arrived + 2)
    mine_uncoded = found[0, 0] > 0
    forward(arrived + 3)

    @pl.when(mine_uncoded)
    def _():
        @pl.loop(0, UNITS)
        def _(j):
            tx[raw_at(j)] = _high_bytes(*_to_pairs(x_ref[rows(8 * j), :]))

    def wait_group(i):
        part = from_x.at[pl.ds(*GROUPS[i])]
        pltpu.make_async_copy(part, part, x_sems.at[i]).wait()

    def decode(decoder, high, cycles):
        while decoder.left:
            cycles -= 17 + 0.85 * _live(decoder.left - 1)
            if cycles < 0:
                break
            j, hu, hv = decoder.pop()
            high[2 * j], high[2 * j + 1] = hu, hv

    for p in range(arrived + 4, WIRE):
        forward(p)
        for _ in range(3):
            if sent < min(WIRE, p + LEAD):
                y_copy(sent).start()
                sent += 1
        if p == EARLY:
            load_other.wait()

            @pl.when(my_x == 0)
            def _():
                for i in range(EXTRA):
                    pairs = _to_pairs(x_ref[rows(M - 8 * (EXTRA - i)), :])
                    tx[WIRE + i] = _low_bytes(*pairs)

        if sent == WIRE:
            sent += EXTRA

            @pl.when(my_x == 0)
            def _():
                for i, (start, size) in enumerate(GROUPS):
                    if start >= SPLIT:
                        src, dst = tx.at[pl.ds(start + EXTRA, size)], from_x.at[pl.ds(start, size)]
                        remote(src, dst, y_sent, x_sems.at[i], y_peer).start()

            @pl.when(mine_uncoded)
            def _():
                for i in range(len(RAW_PARTS)):
                    raw_copy(i, 0).start()

        if p == HEADER + 1:
            found = misfits(from_y)
        elif p == HEADER + 2:
            y_uncoded = found[0, 0] > 0
        elif p == LATE - 1:
            y_decoder = _Decoder(from_y, y_uncoded)
        elif LATE <= p < OTHER_AT:
            decode(y_decoder, high_y, SLOT)
        elif p == OTHER_AT:
            wait_group(0)
            found = misfits(from_x)
        elif p == OTHER_AT + 1:
            x_uncoded = found[0, 0] > 0
        elif p == OTHER_AT + 2:
            x_decoder = _Decoder(from_x, x_uncoded)
        elif p > OTHER_AT + 2:
            decode(x_decoder, high_x, SLOT)
    assert sent == WIRE + EXTRA
    decode(y_decoder, high_y, np.inf)
    decode(x_decoder, high_x, np.inf)

    def use_raw(wire, high):
        @pl.loop(0, UNITS)
        def _(j):
            raw = wire[raw_at(j)]
            high[2 * j] = _shl(raw & EVEN, 8) - BORROW
            high[2 * j + 1] = (raw & ODD) - BORROW

    @pl.when(mine_uncoded | y_uncoded | x_uncoded)
    def _():
        @pl.when(y_uncoded)
        def _():
            for i in range(len(RAW_PARTS)):
                raw_copy(i, 0).wait_recv()
                raw_copy(i, 1).start()
            use_raw(from_y, high_y)

        @pl.when(x_uncoded)
        def _():
            for i in range(len(RAW_PARTS)):
                raw_copy(i, 1).wait_recv()
            use_raw(from_x, high_x)

        for hop, uncoded in enumerate((mine_uncoded, y_uncoded)):

            @pl.when(uncoded)
            def _():
                for i in range(len(RAW_PARTS)):
                    raw_copy(i, hop).wait_send()

    def add(j, decoder, high, x_row, out_row):
        pairs = decoder.join(high[2 * j], high[2 * j + 1], decoder.wire[_wire(j)])
        total = x_ref[rows(x_row + 8 * j), :] + _from_pairs(*pairs)
        out_ref[rows(out_row + 8 * j), :] = total.astype(out_ref.dtype)

    def wait_sent(y_units, x_units):
        y_part, x_part = pl.ds(0, y_units), pl.ds(0, x_units)
        remote(tx.at[y_part], tx.at[y_part], y_sent, y_sent, y_peer).wait_send()
        remote(from_y.at[x_part], from_y.at[x_part], x_sent, x_sent, x_peer).wait_send()

    for j in range(UNITS):
        add(j, y_decoder, high_y, 0, mine)
    for j in range(EARLY):
        add(j, x_decoder, high_x, HALF, other)
    order = sorted(range(1, len(GROUPS)), key=lambda i: GROUP_ENDS[i] - EXTRA * (GROUP_ENDS[i] > SPLIT))
    for i in order:
        if i == order[-2]:
            pl.when(my_x == 0)(lambda: wait_sent(WIRE + EXTRA, WIRE))
            pl.when(my_x == 1)(lambda: wait_sent(WIRE, SPLIT))
        wait_group(i)
        start, size = GROUPS[i]
        for p in range(start, start + size):
            add(p - LATE + EARLY, x_decoder, high_x, HALF, other)


def pallas_dist_ar_xy_y_m1024_n512_kernel(x: jax.Array):
    def units(n):
        return pltpu.VMEM((n, 8, 128), jnp.int32)

    dma = pltpu.SemaphoreType.DMA
    return pl.pallas_call(
        _kernel,
        out_shape=jax.ShapeDtypeStruct((M, N), jnp.bfloat16),
        in_specs=[pl.BlockSpec(memory_space=pltpu.HBM)],
        out_specs=pl.BlockSpec(memory_space=pltpu.VMEM),
        scratch_shapes=[
            pltpu.VMEM((M, N), jnp.float32),
            *(units(RAW + UNITS - FULL) for _ in range(3)),
            *(units(2 * UNITS) for _ in range(2)),
            dma((len(LOADS) + 1,)),
            dma,
            dma,
            dma((WIRE,)),
            dma((len(GROUPS),)),
            dma((4 * len(RAW_PARTS),)),
            pltpu.SemaphoreType.REGULAR,
        ],
        compiler_params=pltpu.CompilerParams(
            collective_id=0, disable_bounds_checks=True, disable_semaphore_checks=True
        ),
    )(x)
```

```python
import jax
import jax.numpy as jnp
import numpy as np
from jax import lax
from jax.experimental import pallas as pl
from jax.experimental.pallas import tpu as pltpu

M, N = 1024, 512
HALF = M // 2
UNITS = HALF // 8

WORDS = 9
FULL = 5
POOL = 10
HEAD_ROW = 16 - (2 + POOL)
STACK = 2
PREFIXES = STACK + FULL
MANTISSAS = PREFIXES + UNITS // 4
END = MANTISSAS + UNITS
EXTRA = 10
SPLIT = END - EXTRA
RAW = END + EXTRA
RAW_PAIRS = (UNITS - FULL + 1) // 2

EARLY = 16
LATE = MANTISSAS + EARLY
SEND_ORDER = (
    *range(MANTISSAS, LATE), *range(PREFIXES, MANTISSAS), *range(PREFIXES), *range(LATE, END)
)
LOADS = (1, 1, 2) + (4,) * 15
GREET = 24
FIRST_FORWARDS = (51, 55, 59, 63)
LEAD = 28
OTHER_AT = 58
DECODES = 3
GROUP_ENDS = (LATE, 55, 67, 71, 74, 76, SPLIT, SPLIT + 4, SPLIT + 7, SPLIT + 9, END)


def _i32(bits):
    return np.uint32(bits).astype(np.int32)


def _bytes(b):
    return _i32(b * 0x01010101)


EVEN, ODD = _i32(0x00FF00FF), _i32(0xFF00FF00)
SIGN, MANTISSA, BORROW = _i32(0x80008000), _i32(0x007F007F), _i32(0x00800080)


def _shl(a, n):
    return lax.shift_left(a, jnp.broadcast_to(n, a.shape))


def _shr(a, n):
    return lax.shift_right_logical(a, jnp.broadcast_to(n, a.shape))


def _at_least(a, c):
    return (a + _bytes(0x80 - c)) & _bytes(0x80)


def _span(start, stop):
    first = max(8 * start, HEAD_ROW)
    return pl.ds(first, 8 * stop - first)


def _live(j):
    n = 4 * (j + 1)
    return min(j + 1, WORDS, int(np.ceil((0.58 * n + 7.2 * np.sqrt(n) + 16) / 32)))


def _to_pairs(rows):
    tiles = [rows[:, c : c + 128] for c in range(0, N, 128)]
    return tuple(
        pltpu.bitcast(jnp.concatenate(tiles[i : i + 2], axis=0).astype(jnp.bfloat16), jnp.int32)
        for i in (0, 2)
    )


def _from_pairs(u, v):
    u, v = (pltpu.bitcast(w, jnp.bfloat16).astype(jnp.float32) for w in (u, v))
    return jnp.concatenate([u[:8], u[8:], v[:8], v[8:]], axis=1)


def _mantissas(u, v):
    return ((u & MANTISSA) | _shr(u & SIGN, 8)) | (_shl(v & MANTISSA, 8) | (v & SIGN))


def _exponents(u, v):
    return (_shr(u, 7) & EVEN) | (_shl(v, 1) & ODD)


def _reference(pairs):
    total = sum((w & 0x7FFF) + (_shr(w, 16) & 0x7FFF) for w in pairs).astype(jnp.float32)
    total = jnp.sum(jnp.sum(total, axis=1, keepdims=True), axis=0, keepdims=True)
    mean = jnp.broadcast_to(total, (8, 128)) * (1.0 / (2048 * len(pairs)))
    return jnp.minimum(mean.astype(jnp.int32) + 532, 0x7FFF)


def _sublane():
    return lax.broadcasted_iota(jnp.int32, (8, 128), 0)


def _or_sublanes(a):
    for shift in (4, 2, 1):
        a = a | pltpu.roll(a, shift, 0)
    return a


def _pool_rows(wanted):
    one = jnp.ones_like(wanted)
    return [
        lax.population_count(wanted & (_shl(one, _sublane() + 8 * i) - 1))
        for i in range(WORDS - FULL)
    ]


class _Encoder:
    def __init__(self, k):
        self.k = k
        self.k2 = k | _shl(k, 16) | SIGN
        zero = jnp.zeros_like(k)
        self.words = None
        self.bits, self.room, self.long, self.below_k = zero, zero, zero, ~zero

    def push(self, j, u, v):
        u, v = self.k2 - (u & ~SIGN), self.k2 - (v & ~SIGN)
        d = _exponents(u, v)
        lt1, lt2 = _at_least(d, 1) ^ _bytes(0x80), _at_least(d, 2) ^ _bytes(0x80)
        ge5 = _at_least(d, 5)
        stacked = _shr(lt2 | ge5, 7)
        prefix = ((d + _bytes(2)) & _bytes(3)) | stacked | _shl(stacked, 1)
        size = ((d + _bytes(0x7C)) & (ge5 - _shr(ge5, 7))) + _shr(_at_least(d, 8), 7)
        size += _shr(_at_least(d, 19), 7) + _shr(lt2, 5) + _shr(lt1, 4) + _shr(lt1, 5)
        end = size + _shl(size, 8)
        end = end + _shl(end, 16)
        code = ((stacked & 1) | _shl(_shr(stacked, 8) & 1, end & 31)) | (
            _shl(_shr(stacked, 16) & 1, _shr(end, 8) & 31)
            | _shl(_shr(stacked, 24), _shr(end, 16) & 31)
        )
        self.below_k &= u & v
        self.long |= (_shr(d, 1) & _bytes(0x60)) | end
        self.bits += _shr(end, 24)
        if j == UNITS - 1 or _live(j + 1) != _live(j):
            self.room |= 32 * _live(j) - self.bits
        n = _shr(end, 24) & 31
        if j == 0:
            self.words = _shl(_shl(code, 1), n ^ 31)[None]
        else:
            old, kept = self.words, _shr(self.words, n)
            if _live(j) > old.shape[0]:
                kept = jnp.concatenate([kept, jnp.zeros_like(code)[None]])
            above = jnp.concatenate([code[None], old])[: _live(j)]
            self.words = kept | _shl(_shl(above, 1), n ^ 31)
        return _shl(prefix, 2 * (j % 4))

    def header(self):
        misfit = (self.long & _bytes(0xE0)) | (~self.below_k & SIGN)
        misfit = jnp.where((misfit != 0) | (self.room < 0), 1, 0)
        fills = [self.bits > 32 * i for i in range(FULL, WORDS)]
        one = jnp.ones_like(misfit)
        wanted = sum(
            jnp.where(f, _shl(one, _sublane() + 8 * i), 0) for i, f in enumerate(fills)
        )
        wanted = _or_sublanes(wanted)
        misfit = _or_sublanes(misfit) | jnp.where(lax.population_count(wanted) > POOL, 1, 0)
        places = _pool_rows(wanted)
        rows = [self.k | _shl(misfit, 15), wanted]
        for row in range(POOL):
            word = sum(
                jnp.where(f & (place == row), self.words[FULL + i], 0)
                for i, (f, place) in enumerate(zip(fills, places))
            )
            rows.append(_or_sublanes(word))
        tiles = [wanted, wanted]
        for i, row in enumerate(rows, HEAD_ROW):
            tiles[i // 8] = jnp.where(_sublane() == i % 8, row, tiles[i // 8])
        return jnp.concatenate(tiles)


class _Decoder:
    def __init__(self, wire, uncoded):
        self.wire = wire

        def row(i):
            return jnp.broadcast_to(wire[pl.ds(HEAD_ROW + i, 1), :], (8, 128))

        k = row(0)
        places = _pool_rows(row(1))
        pooled = [k] * len(places)
        for i in range(POOL):
            word = row(2 + i)
            pooled = [jnp.where(place == i, word, w) for place, w in zip(places, pooled)]
        self.words = jnp.stack([wire[_span(p, p + 1), :] for p in range(STACK, PREFIXES)] + pooled)
        self.coded = jnp.where(uncoded, 0, jnp.full_like(k, _bytes(1)))
        k = jnp.where(uncoded, 0x7F, k & 0x7FFF)
        high, low = _shl(_shr(k, 7) - 1, 7), (k & 0x7F) | 0x80
        self.k_high, self.k_low = high + _shl(high, 16), low | _shl(low, 16)
        self.left = UNITS
        self._scan()

    def _scan(self):
        j = self.left - 1
        prefix = _shr(self.wire[_span(PREFIXES + j // 4, PREFIXES + j // 4 + 1), :], 2 * (j % 4))
        self.prefix, self.stacked = prefix & _bytes(3), prefix & _shr(prefix, 1) & self.coded
        word, self.sizes = self.words[0], []
        for i in (3, 2, 1, 0):
            size = jnp.where(self.stacked & (1 << 8 * i) != 0, lax.clz(word) + 1, 0)
            self.sizes.append(size)
            word = _shl(word, size)

    def pop(self):
        j = self.left = self.left - 1
        (n3, n2, n1, n0), prefix, stacked = self.sizes, self.prefix, self.stacked
        if j:
            n = n3 + n2 + n1 + n0
            old, live = self.words, _live(j - 1)
            self.words = _shl(old[:live], n)
            if old.shape[0] > 1:
                below = _shr(_shr(old[1 : live + 1], 1), n ^ 31)
                if below.shape[0] < live:
                    below = jnp.concatenate([below, jnp.zeros_like(n)[None]])
                self.words |= below
            self._scan()
        size = (n0 | _shl(n1, 8)) | (_shl(n2, 16) | _shl(n3, 24))
        ge4, ge5, ge16, ge17 = (_at_least(size, c) for c in (4, 5, 16, 17))
        is4, is16 = ge4 ^ ge5, ge16 ^ ge17
        d = prefix + _bytes(2) + size - stacked - _shr(ge5, 7) - _shr(ge17, 7)
        d = (d + _shr(is4, 7) - _shr(is4, 4)) & ~(is16 - _shr(is16, 7))
        return j, self.k_high - _shl(d & EVEN, 7), self.k_high - _shr(d & ODD, 1)

    def join(self, j, eu, ev):
        low = self.wire[_span(MANTISSAS + j, MANTISSAS + j + 1), :]
        mu, mv = low & MANTISSA, _shr(low, 8) & MANTISSA
        return (
            eu + (mu | (_shl(low, 8) & SIGN)) + ((self.k_low - mu) & BORROW),
            ev + (mv | (low & SIGN)) + ((self.k_low - mv) & BORROW),
        )


def _kernel(
    x_hbm, out_ref, x_ref, tx, from_y, from_x, exp_y, exp_x,
    load_sems, y_sent, x_sent, y_sems, x_sems, raw_sems, x_started,
):
    my_x, my_y = lax.axis_index("x"), lax.axis_index("y")
    y_peer, x_peer = (my_x, 1 - my_y), (1 - my_x, my_y)
    mine, other = my_x * UNITS, (1 - my_x) * UNITS

    def rows(unit, count=1):
        start = 8 * unit
        return pl.ds(start if isinstance(start, int) else pl.multiple_of(start, 8), 8 * count)

    def remote(src, dst, send_sem, recv_sem, peer):
        return pltpu.make_async_remote_copy(
            src, dst, send_sem, recv_sem, device_id=peer, device_id_type=pl.DeviceIdType.MESH
        )

    def signal(sem, peer):
        pl.semaphore_signal(sem, inc=1, device_id=peer, device_id_type=pl.DeviceIdType.MESH)

    def y_copy(p):
        part = _span(SEND_ORDER[p], SEND_ORDER[p] + 1)
        return remote(tx.at[part], from_y.at[part], y_sent, y_sems.at[p], y_peer)

    def x_copy(p):
        part = _span(SEND_ORDER[p], SEND_ORDER[p] + 1)
        group = sum(p >= end for end in GROUP_ENDS)
        return remote(from_y.at[part], from_x.at[part], x_sent, x_sems.at[group], x_peer)

    def raw_y_copy(i, pairs=1):
        part = rows(RAW + 2 * i, 2 * pairs)
        return remote(tx.at[part], from_y.at[part], raw_sems.at[0], raw_sems.at[3 + i], y_peer)

    def raw_x_copy(i, pairs=1):
        part = rows(RAW + 2 * i, 2 * pairs)
        return remote(from_y.at[part], from_x.at[part], raw_sems.at[1], raw_sems.at[2], x_peer)

    def raw_rows(j):
        return rows(jnp.where(j < FULL, STACK + j, RAW + j - FULL))

    def misfits(wire):
        bit = wire[pl.ds(HEAD_ROW, 1), :] & 0x8000
        return jnp.max(bit.astype(jnp.float32), axis=1, keepdims=True)

    barrier = pltpu.get_barrier_semaphore()
    loads, first = {}, 0
    for i, n in enumerate(LOADS):
        loads[first] = pltpu.make_async_copy(
            x_hbm.at[rows(mine + first, n)], x_ref.at[rows(first, n)], load_sems.at[i]
        )
        loads[first].start()
        first += n
        if i == 0:
            signal(barrier, y_peer)
            pl.when(my_x == 0)(lambda: signal(barrier, x_peer))
    load_other = pltpu.make_async_copy(
        x_hbm.at[rows(other, UNITS)], x_ref.at[rows(UNITS, UNITS)], load_sems.at[len(LOADS)]
    )
    load_other.start()

    def greet():
        pl.semaphore_wait(barrier, 1 + my_x)
        y_copy(0).start()
        pl.when(my_x == 1)(lambda: signal(x_started, x_peer))

    def forward(p):
        y_copy(p).wait_recv()
        if p == 0:
            pl.when(my_x == 0)(lambda: pl.semaphore_wait(x_started, 1))
        if p < SPLIT:
            x_copy(p).start()
        else:
            pl.when(my_x == 0)(lambda: x_copy(p).start())

    sent = arrived = 0
    todo = []
    for j in range(UNITS):
        if j in loads:
            loads[j].wait()
        u, v = _to_pairs(x_ref[rows(j), :])
        tx[rows(MANTISSAS + j), :] = _mantissas(u, v)
        if j < EARLY:
            pl.when(my_y == 1)(greet if j == 0 else lambda: y_copy(j).start())
            sent += 1
        if j == GREET - 1:

            @pl.when(my_y == 0)
            def _():
                greet()
                for p in range(1, sent):
                    y_copy(p).start()

        todo.append((j, u, v))
        if j == 1:
            encoder = _Encoder(_reference([w for _, *pair in todo for w in pair]))
        while j >= 1 and todo:
            i, u, v = todo.pop(0)
            placed = encoder.push(i, u, v)
            prefixes = prefixes | placed if i % 4 else placed
            if i % 4 == 3:
                tx[rows(PREFIXES + i // 4), :] = prefixes
        while j >= GREET and sent < EARLY + (j + 1) // 4:
            y_copy(sent).start()
            sent += 1
        if j in FIRST_FORWARDS:
            forward(arrived)
            arrived += 1
    for i in range(FULL):
        tx[rows(STACK + i), :] = encoder.words[i]
    forward(arrived)
    tx[rows(0, 2), :] = encoder.header()
    forward(arrived + 1)
    found = misfits(tx)
    forward(arrived + 2)
    mine_uncoded = found[0, 0] > 0
    forward(arrived + 3)

    @pl.when(mine_uncoded)
    def _():
        @pl.loop(0, FULL + 2 * RAW_PAIRS)
        def _(j):
            tx[raw_rows(j), :] = _exponents(*_to_pairs(x_ref[rows(jnp.minimum(j, UNITS - 1)), :]))

    def wait_group(i):
        part = from_x.at[_span(GROUP_ENDS[i - 1] if i else 0, GROUP_ENDS[i])]
        pltpu.make_async_copy(part, part, x_sems.at[i]).wait()

    decoders = []

    def decode(count):
        for decoder, exp in zip(decoders, (exp_y, exp_x)):
            while decoder.left and count:
                count -= 1
                j, eu, ev = decoder.pop()
                exp[2 * j], exp[2 * j + 1] = eu, ev

    for p in range(arrived + 4, END):
        forward(p)
        for _ in range(3):
            if sent < min(END, p + LEAD):
                y_copy(sent).start()
                sent += 1
        if sent == END:
            sent += EXTRA

            @pl.when(my_x == 0)
            def _():
                for i, (start, stop) in enumerate(zip(GROUP_ENDS, GROUP_ENDS[1:]), 1):
                    if start >= SPLIT:
                        src, dst = tx.at[_span(start + EXTRA, stop + EXTRA)], _span(start, stop)
                        remote(src, from_x.at[dst], y_sent, x_sems.at[i], y_peer).start()

            @pl.when(mine_uncoded)
            def _():
                pl.loop(0, RAW_PAIRS)(lambda i: raw_y_copy(i).start())

        if p == 24:
            load_other.wait()

            @pl.when(my_x == 0)
            def _():
                for i in range(EXTRA):
                    pairs = _to_pairs(x_ref[rows(2 * UNITS - EXTRA + i), :])
                    tx[rows(END + i), :] = _mantissas(*pairs)

        elif p == SEND_ORDER.index(1):
            found = misfits(from_y)
        elif p == SEND_ORDER.index(1) + 1:
            y_uncoded = found[0, 0] > 0
        elif p == LATE - 1:
            decoders.append(_Decoder(from_y, y_uncoded))
        elif p == OTHER_AT:
            wait_group(0)
            found = misfits(from_x)
        elif p == OTHER_AT + 1:
            x_uncoded = found[0, 0] > 0
        elif p == OTHER_AT + 2:
            decoders.append(_Decoder(from_x, x_uncoded))
        else:
            decode(DECODES)
    assert sent == END + EXTRA
    decode(2 * UNITS)

    def use_raw(wire, exp):
        @pl.loop(0, UNITS)
        def _(j):
            raw = wire[raw_rows(j), :]
            exp[2 * j] = _shl(raw & EVEN, 7) - BORROW
            exp[2 * j + 1] = _shr(raw & ODD, 1) - BORROW

    @pl.when(mine_uncoded | y_uncoded | x_uncoded)
    def _():
        @pl.when(y_uncoded)
        def _():
            @pl.loop(0, RAW_PAIRS)
            def _(i):
                raw_y_copy(i).wait_recv()
                raw_x_copy(i).start()

            use_raw(from_y, exp_y)
            raw_x_copy(0, RAW_PAIRS).wait_send()

        @pl.when(x_uncoded)
        def _():
            raw_x_copy(0, RAW_PAIRS).wait_recv()
            use_raw(from_x, exp_x)

        pl.when(mine_uncoded)(lambda: raw_y_copy(0, RAW_PAIRS).wait_send())

    def add(j, half):
        exp = (exp_y, exp_x)[half]
        partner = _from_pairs(*decoders[half].join(j, exp[2 * j], exp[2 * j + 1]))
        total = x_ref[rows(half * UNITS + j), :] + partner
        out_ref[rows((mine, other)[half] + j), :] = total.astype(out_ref.dtype)

    def wait_sent(y_units, x_units):
        y_part, x_part = _span(0, y_units), _span(0, x_units)
        remote(tx.at[y_part], from_y.at[y_part], y_sent, y_sems.at[0], y_peer).wait_send()
        remote(from_y.at[x_part], from_x.at[x_part], x_sent, x_sems.at[0], x_peer).wait_send()

    for j in range(UNITS):
        add(j, 0)
    for j in range(EARLY):
        add(j, 1)
    order = sorted(
        range(1, len(GROUP_ENDS)), key=lambda i: GROUP_ENDS[i] - EXTRA * (GROUP_ENDS[i] > SPLIT)
    )
    for i in order:
        if i == order[-2]:
            pl.when(my_x == 0)(lambda: wait_sent(END + EXTRA, END))
            pl.when(my_x == 1)(lambda: wait_sent(END, SPLIT))
        wait_group(i)
        for unit in range(GROUP_ENDS[i - 1], GROUP_ENDS[i]):
            add(unit - MANTISSAS, 1)


def pallas_dist_ar_xy_y_m1024_n512_kernel(x: jax.Array):
    dma = pltpu.SemaphoreType.DMA
    return pl.pallas_call(
        _kernel,
        out_shape=jax.ShapeDtypeStruct((M, N), jnp.bfloat16),
        in_specs=[pl.BlockSpec(memory_space=pltpu.HBM)],
        out_specs=pl.BlockSpec(memory_space=pltpu.VMEM),
        scratch_shapes=[
            pltpu.VMEM((M, N), jnp.float32),
            *(pltpu.VMEM((8 * (RAW + 2 * RAW_PAIRS), 128), jnp.int32) for _ in range(3)),
            *(pltpu.VMEM((2 * UNITS, 8, 128), jnp.int32) for _ in range(2)),
            dma((len(LOADS) + 1,)),
            dma,
            dma,
            dma((END,)),
            dma((len(GROUP_ENDS),)),
            dma((3 + RAW_PAIRS,)),
            pltpu.SemaphoreType.REGULAR,
        ],
        compiler_params=pltpu.CompilerParams(
            collective_id=0, disable_bounds_checks=True, disable_semaphore_checks=True
        ),
    )(x)
```

```python
import jax
import jax.numpy as jnp
import numpy as np
from jax import lax
from jax.experimental import pallas as pl
from jax.experimental.pallas import tpu as pltpu

M, N = 1024, 512
HALF = M // 2
UNITS = HALF // 8

WORDS = 9
FULL = 5
POOL = 10
HEAD_ROW = 16 - (2 + POOL)
STACK = 2
PREFIXES = STACK + FULL
MANTISSAS = PREFIXES + UNITS // 4
END = MANTISSAS + UNITS
EXTRA = 10
SPLIT = END - EXTRA
RAW = END + EXTRA
RAW_PAIRS = (UNITS - FULL + 1) // 2

EARLY = 16
LATE = MANTISSAS + EARLY
SEND_ORDER = (
    *range(MANTISSAS, LATE), *range(PREFIXES, MANTISSAS), *range(PREFIXES), *range(LATE, END)
)
LOADS = (1, 1, 2) + (4,) * 15
GREET = 28
FIRST_FORWARD = 52
LEAD = 28
OTHER_AT = 58
DECODES = 3
GROUP_ENDS = (LATE, 55, 67, 71, 74, 76, SPLIT, SPLIT + 4, SPLIT + 7, SPLIT + 9, END)


def _i32(bits):
    return np.uint32(bits).astype(np.int32)


def _bytes(b):
    return _i32(b * 0x01010101)


EVEN, ODD = _i32(0x00FF00FF), _i32(0xFF00FF00)
SIGN, MANTISSA, BORROW = _i32(0x80008000), _i32(0x007F007F), _i32(0x00800080)


def _shl(a, n):
    return lax.shift_left(a, np.int32(n) if isinstance(n, int) else n)


def _shr(a, n):
    return lax.shift_right_logical(a, np.int32(n) if isinstance(n, int) else n)


def _at_least(a, c):
    return (a + _bytes(0x80 - c)) & _bytes(0x80)


def _span(start, stop):
    first = max(8 * start, HEAD_ROW)
    return pl.ds(first, 8 * stop - first)


def _live(j):
    n = 4 * (j + 1)
    return min(j + 1, WORDS, int(np.ceil((0.58 * n + 7.2 * np.sqrt(n) + 16) / 32)))


def _to_pairs(rows):
    tiles = [rows[:, c : c + 128].reshape(-1, 8, 128) for c in range(0, N, 128)]
    pairs = (jnp.concatenate(tiles[i : i + 2], axis=1).reshape(-1, 128) for i in (0, 2))
    return tuple(pltpu.bitcast(p.astype(jnp.bfloat16), jnp.int32) for p in pairs)


def _from_pairs(u, v):
    pairs = (pltpu.bitcast(w, jnp.bfloat16).astype(jnp.float32) for w in (u, v))
    tiles = [p.reshape(-1, 16, 128)[:, r : r + 8] for p in pairs for r in (0, 8)]
    return jnp.concatenate([t.reshape(-1, 128) for t in tiles], axis=1)


def _mantissas(u, v):
    return ((u & MANTISSA) | _shr(u & SIGN, 8)) | (_shl(v & MANTISSA, 8) | (v & SIGN))


def _exponents(u, v):
    return (_shr(u, 7) & EVEN) | (_shl(v, 1) & ODD)


def _reference(pairs):
    total = sum((w & 0x7FFF) + (_shr(w, 16) & 0x7FFF) for w in pairs).astype(jnp.float32)
    total = jnp.sum(jnp.sum(total, axis=1, keepdims=True), axis=0, keepdims=True)
    mean = jnp.broadcast_to(total, (8, 128)) * (1.0 / (2 * sum(w.size for w in pairs)))
    return jnp.minimum(mean.astype(jnp.int32) + 532, 0x7FFF)


def _sublane():
    return lax.broadcasted_iota(jnp.int32, (8, 128), 0)


def _or_sublanes(a):
    for shift in (4, 2, 1):
        a = a | pltpu.roll(a, shift, 0)
    return a


def _pool_rows(wanted):
    one = jnp.ones_like(wanted)
    return [
        lax.population_count(wanted & (_shl(one, _sublane() + 8 * i) - 1))
        for i in range(WORDS - FULL)
    ]


class _Encoder:
    def __init__(self, k):
        self.k = k
        self.k2 = k | _shl(k, 16) | SIGN
        zero = jnp.zeros_like(k)
        self.words = None
        self.bits, self.room, self.long, self.below_k = zero, zero, zero, ~zero

    def push(self, first, u, v):
        u, v = (self.k2[None] - (w.reshape(-1, 8, 128) & ~SIGN) for w in (u, v))
        d = _exponents(u, v)
        lt1, lt2 = _at_least(d, 1) ^ _bytes(0x80), _at_least(d, 2) ^ _bytes(0x80)
        ge5 = _at_least(d, 5)
        stacked = _shr(lt2 | ge5, 7)
        size = ((d + _bytes(0x7C)) & (ge5 - _shr(ge5, 7))) + _shr(_at_least(d, 8), 7)
        size += _shr(_at_least(d, 19), 7) + _shr(lt2, 5) + _shr(lt1, 4) + _shr(lt1, 5)
        end = size + _shl(size, 8)
        end = end + _shl(end, 16)
        code = ((stacked & 1) | _shl(_shr(stacked, 8) & 1, end & 31)) | (
            _shl(_shr(stacked, 16) & 1, _shr(end, 8) & 31)
            | _shl(_shr(stacked, 24), _shr(end, 16) & 31)
        )
        below_k, long, bits = u & v, (_shr(d, 1) & _bytes(0x60)) | end, _shr(end, 24)
        for i, j in enumerate(range(first, first + d.shape[0])):
            self.below_k &= below_k[i]
            self.long |= long[i]
            self.bits += bits[i]
            if j == UNITS - 1 or _live(j + 1) != _live(j):
                self.room |= 32 * _live(j) - self.bits
            n, new = bits[i : i + 1] & 31, code[i : i + 1]
            if j == 0:
                self.words = _shl(_shl(new, 1), n ^ 31)
                continue
            old, kept = self.words, _shr(self.words, n)
            if _live(j) > old.shape[0]:
                kept = jnp.concatenate([kept, jnp.zeros_like(new)])
            above = jnp.concatenate([new, old])[: _live(j)]
            self.words = kept | _shl(_shl(above, 1), n ^ 31)
        return ((d + _bytes(2)) & _bytes(3)) | stacked | _shl(stacked, 1)

    def header(self):
        misfit = (self.long & _bytes(0xE0)) | (~self.below_k & SIGN)
        misfit = jnp.where((misfit != 0) | (self.room < 0), 1, 0)
        fills = [self.bits > 32 * i for i in range(FULL, WORDS)]
        one = jnp.ones_like(misfit)
        wanted = sum(
            jnp.where(f, _shl(one, _sublane() + 8 * i), 0) for i, f in enumerate(fills)
        )
        wanted = _or_sublanes(wanted)
        misfit = _or_sublanes(misfit) | jnp.where(lax.population_count(wanted) > POOL, 1, 0)
        places = _pool_rows(wanted)
        rows = [self.k | _shl(misfit, 15), wanted]
        for row in range(POOL):
            word = sum(
                jnp.where(f & (place == row), self.words[FULL + i], 0)
                for i, (f, place) in enumerate(zip(fills, places))
            )
            rows.append(_or_sublanes(word))
        tiles = [wanted, wanted]
        for i, row in enumerate(rows, HEAD_ROW):
            tiles[i // 8] = jnp.where(_sublane() == i % 8, row, tiles[i // 8])
        return jnp.concatenate(tiles)


class _Decoder:
    def __init__(self, wire, uncoded):
        self.wire = wire

        def row(i):
            return jnp.broadcast_to(wire[pl.ds(HEAD_ROW + i, 1), :], (8, 128))

        k = row(0)
        places = _pool_rows(row(1))
        pooled = [k] * len(places)
        for i in range(POOL):
            word = row(2 + i)
            pooled = [jnp.where(place == i, word, w) for place, w in zip(places, pooled)]
        self.words = jnp.stack([wire[_span(p, p + 1), :] for p in range(STACK, PREFIXES)] + pooled)
        self.coded = jnp.where(uncoded, 0, jnp.full_like(k, _bytes(1)))
        k = jnp.where(uncoded, 0x7F, k & 0x7FFF)
        high, low = _shl(_shr(k, 7) - 1, 7), (k & 0x7F) | 0x80
        self.k_high, self.k_low = high + _shl(high, 16), low | _shl(low, 16)
        self.left = UNITS
        self._scan()

    def _scan(self):
        j = self.left - 1
        prefix = _shr(self.wire[_span(PREFIXES + j // 4, PREFIXES + j // 4 + 1), :], 2 * (j % 4))
        self.prefix, self.stacked = prefix, prefix & _shr(prefix, 1) & self.coded
        word, self.sizes = self.words[0], []
        for i in (3, 2, 1, 0):
            stacked = self.stacked & (1 << 8 * i)
            self.sizes.append(lax.select(stacked != 0, lax.clz(word) + 1, stacked))
            if i:
                word = _shl(word, self.sizes[-1])

    def pop(self, count):
        popped = []
        for _ in range(count):
            j = self.left = self.left - 1
            popped.insert(0, (*self.sizes, self.prefix, self.stacked))
            if j:
                n = ((self.sizes[0] + self.sizes[1]) + self.sizes[2] + self.sizes[3])[None]
                old, live = self.words, _live(j - 1)
                self.words = _shl(old[:live], n)
                below = _shr(_shr(old[1 : live + 1], 1), n ^ 31)
                if below.shape[0] < live:
                    below = jnp.concatenate([below, jnp.zeros_like(n)])
                self.words |= below
                self._scan()
        n3, n2, n1, n0, prefix, stacked = (jnp.stack(a) for a in zip(*popped))
        size = (n0 | _shl(n1, 8)) | (_shl(n2, 16) | _shl(n3, 24))
        ge4, ge5, ge16, ge17 = (_at_least(size, c) for c in (4, 5, 16, 17))
        is4, is16 = ge4 ^ ge5, ge16 ^ ge17
        d = (prefix & _bytes(3)) + _bytes(2) + size - stacked - _shr(ge5, 7) - _shr(ge17, 7)
        d = (d + _shr(is4, 7) - _shr(is4, 4)) & ~(is16 - _shr(is16, 7))
        return tuple(
            (self.k_high[None] - e).reshape(-1, 128) for e in (_shl(d & EVEN, 7), _shr(d & ODD, 1))
        )

    def join(self, low, eu, ev):
        k_low = jnp.concatenate([self.k_low] * (low.shape[0] // 8))
        mu, mv = low & MANTISSA, _shr(low, 8) & MANTISSA
        return (
            eu + (mu | (_shl(low, 8) & SIGN)) + ((k_low - mu) & BORROW),
            ev + (mv | (low & SIGN)) + ((k_low - mv) & BORROW),
        )


def _kernel(
    x_hbm, out_ref, x_ref, tx, from_y, from_x, exp_y, exp_x,
    load_sems, y_sent, x_sent, y_sems, x_sems, raw_sems, x_started,
):
    my_x, my_y = lax.axis_index("x"), lax.axis_index("y")
    y_peer, x_peer = (my_x, 1 - my_y), (1 - my_x, my_y)
    mine, other = my_x * UNITS, (1 - my_x) * UNITS

    def rows(unit, count=1):
        start = 8 * unit
        return pl.ds(start if isinstance(start, int) else pl.multiple_of(start, 8), 8 * count)

    def remote(src, dst, send_sem, recv_sem, peer):
        return pltpu.make_async_remote_copy(
            src, dst, send_sem, recv_sem, device_id=peer, device_id_type=pl.DeviceIdType.MESH
        )

    def signal(sem, peer):
        pl.semaphore_signal(sem, inc=1, device_id=peer, device_id_type=pl.DeviceIdType.MESH)

    def y_copy(p):
        part = _span(SEND_ORDER[p], SEND_ORDER[p] + 1)
        return remote(tx.at[part], from_y.at[part], y_sent, y_sems.at[p], y_peer)

    def x_copy(p):
        part = _span(SEND_ORDER[p], SEND_ORDER[p] + 1)
        group = sum(p >= end for end in GROUP_ENDS)
        return remote(from_y.at[part], from_x.at[part], x_sent, x_sems.at[group], x_peer)

    def raw_y_copy(i, pairs=1):
        part = rows(RAW + 2 * i, 2 * pairs)
        return remote(tx.at[part], from_y.at[part], raw_sems.at[0], raw_sems.at[3 + i], y_peer)

    def raw_x_copy(i, pairs=1):
        part = rows(RAW + 2 * i, 2 * pairs)
        return remote(from_y.at[part], from_x.at[part], raw_sems.at[1], raw_sems.at[2], x_peer)

    def raw_rows(j):
        return rows(jnp.where(j < FULL, STACK + j, RAW + j - FULL))

    def misfits(wire):
        bit = wire[pl.ds(HEAD_ROW, 1), :] & 0x8000
        return jnp.max(bit.astype(jnp.float32), axis=1, keepdims=True)

    barrier = pltpu.get_barrier_semaphore()
    loads, first = {}, 0
    for i, n in enumerate(LOADS):
        loads[first] = pltpu.make_async_copy(
            x_hbm.at[rows(mine + first, n)], x_ref.at[rows(first, n)], load_sems.at[i]
        )
        loads[first].start()
        first += n
        if i == 0:
            signal(barrier, y_peer)
            pl.when(my_x == 0)(lambda: signal(barrier, x_peer))
    load_other = pltpu.make_async_copy(
        x_hbm.at[rows(other, UNITS)], x_ref.at[rows(UNITS, UNITS)], load_sems.at[len(LOADS)]
    )
    load_other.start()

    def greet():
        pl.semaphore_wait(barrier, 1 + my_x)
        y_copy(0).start()
        pl.when(my_x == 1)(lambda: signal(x_started, x_peer))

    def forward(p):
        y_copy(p).wait_recv()
        if p == 0:
            pl.when(my_x == 0)(lambda: pl.semaphore_wait(x_started, 1))
        if p < SPLIT:
            x_copy(p).start()
        else:
            pl.when(my_x == 0)(lambda: x_copy(p).start())

    sent = arrived = 0
    todo, prefixes = [], []
    for j, n in zip(loads, LOADS):
        loads[j].wait()
        u, v = _to_pairs(x_ref[rows(j, n), :])
        tx[rows(MANTISSAS + j, n), :] = _mantissas(u, v)
        if j < EARLY:

            @pl.when(my_y == 1)
            def _():
                for p in range(j, j + n):
                    y_copy(p).start() if p else greet()

            sent += n
        if j + n == GREET:

            @pl.when(my_y == 0)
            def _():
                greet()
                for p in range(1, sent):
                    y_copy(p).start()

        todo.append((j, u, v))
        if j == 1:
            encoder = _Encoder(_reference([w for _, *pair in todo for w in pair]))
        while j >= 1 and todo:
            prefixes.append(encoder.push(*todo.pop(0)))
        if (j + n) % 4 == 0:
            four, prefixes = jnp.concatenate(prefixes), []
            tx[rows(PREFIXES + j // 4), :] = (four[0] | _shl(four[1], 2)) | (
                _shl(four[2], 4) | _shl(four[3], 6)
            )
        while j >= GREET and sent < EARLY + (j + n) // 4:
            y_copy(sent).start()
            sent += 1
        if j + n >= FIRST_FORWARD:
            forward(arrived)
            arrived += 1
    for i in range(FULL):
        tx[rows(STACK + i), :] = encoder.words[i]
    forward(arrived)
    tx[rows(0, 2), :] = encoder.header()
    forward(arrived + 1)
    found = misfits(tx)
    forward(arrived + 2)
    mine_uncoded = found[0, 0] > 0
    forward(arrived + 3)

    @pl.when(mine_uncoded)
    def _():
        @pl.loop(0, FULL + 2 * RAW_PAIRS)
        def _(j):
            tx[raw_rows(j), :] = _exponents(*_to_pairs(x_ref[rows(jnp.minimum(j, UNITS - 1)), :]))

    def wait_group(i):
        part = from_x.at[_span(GROUP_ENDS[i - 1] if i else 0, GROUP_ENDS[i])]
        pltpu.make_async_copy(part, part, x_sems.at[i]).wait()

    decoders = []

    def decode(count):
        for decoder, exp in zip(decoders, (exp_y, exp_x)):
            while n := min(decoder.left, count, DECODES):
                count -= n
                eu, ev = decoder.pop(n)
                exp[0, rows(decoder.left, n), :], exp[1, rows(decoder.left, n), :] = eu, ev

    for p in range(arrived + 4, END):
        forward(p)
        for _ in range(3):
            if sent < min(END, p + LEAD):
                y_copy(sent).start()
                sent += 1
        if sent == END:
            sent += EXTRA

            @pl.when(my_x == 0)
            def _():
                for i, (start, stop) in enumerate(zip(GROUP_ENDS, GROUP_ENDS[1:]), 1):
                    if start >= SPLIT:
                        src, dst = tx.at[_span(start + EXTRA, stop + EXTRA)], _span(start, stop)
                        remote(src, from_x.at[dst], y_sent, x_sems.at[i], y_peer).start()

            @pl.when(mine_uncoded)
            def _():
                pl.loop(0, RAW_PAIRS)(lambda i: raw_y_copy(i).start())

        if p == EARLY + 8:
            load_other.wait()

            @pl.when(my_x == 0)
            def _():
                pairs = _to_pairs(x_ref[rows(2 * UNITS - EXTRA, EXTRA), :])
                tx[rows(END, EXTRA), :] = _mantissas(*pairs)

        elif p == SEND_ORDER.index(1):
            found = misfits(from_y)
        elif p == SEND_ORDER.index(1) + 1:
            y_uncoded = found[0, 0] > 0
        elif p == LATE - 1:
            decoders.append(_Decoder(from_y, y_uncoded))
        elif p == OTHER_AT:
            wait_group(0)
            found = misfits(from_x)
        elif p == OTHER_AT + 1:
            x_uncoded = found[0, 0] > 0
        elif p == OTHER_AT + 2:
            decoders.append(_Decoder(from_x, x_uncoded))
        else:
            decode(DECODES)
    assert sent == END + EXTRA
    decode(2 * UNITS)

    def use_raw(wire, exp):
        @pl.loop(0, UNITS)
        def _(j):
            raw = wire[raw_rows(j), :]
            exp[0, rows(j), :] = _shl(raw & EVEN, 7) - BORROW
            exp[1, rows(j), :] = _shr(raw & ODD, 1) - BORROW

    @pl.when(mine_uncoded | y_uncoded | x_uncoded)
    def _():
        @pl.when(y_uncoded)
        def _():
            @pl.loop(0, RAW_PAIRS)
            def _(i):
                raw_y_copy(i).wait_recv()
                raw_x_copy(i).start()

            use_raw(from_y, exp_y)
            raw_x_copy(0, RAW_PAIRS).wait_send()

        @pl.when(x_uncoded)
        def _():
            raw_x_copy(0, RAW_PAIRS).wait_recv()
            use_raw(from_x, exp_x)

        pl.when(mine_uncoded)(lambda: raw_y_copy(0, RAW_PAIRS).wait_send())

    def add(half, start, stop):
        wire, exp, first = ((from_y, exp_y, mine), (from_x, exp_x, other))[half]
        for j in range(start, stop, 4):
            n = min(4, stop - j)
            pairs = decoders[half].join(
                wire[rows(MANTISSAS + j, n), :], exp[0, rows(j, n), :], exp[1, rows(j, n), :]
            )
            total = x_ref[rows(half * UNITS + j, n), :] + _from_pairs(*pairs)
            out_ref[rows(first + j, n), :] = total.astype(out_ref.dtype)

    def wait_sent(y_units, x_units):
        y_part, x_part = _span(0, y_units), _span(0, x_units)
        remote(tx.at[y_part], from_y.at[y_part], y_sent, y_sems.at[0], y_peer).wait_send()
        remote(from_y.at[x_part], from_x.at[x_part], x_sent, x_sems.at[0], x_peer).wait_send()

    add(0, 0, UNITS)
    add(1, 0, EARLY)
    order = sorted(
        range(1, len(GROUP_ENDS)), key=lambda i: GROUP_ENDS[i] - EXTRA * (GROUP_ENDS[i] > SPLIT)
    )
    for i in order:
        if i == order[-2]:
            pl.when(my_x == 0)(lambda: wait_sent(END + EXTRA, END))
            pl.when(my_x == 1)(lambda: wait_sent(END, SPLIT))
        wait_group(i)
        add(1, GROUP_ENDS[i - 1] - MANTISSAS, GROUP_ENDS[i] - MANTISSAS)


def pallas_dist_ar_xy_y_m1024_n512_kernel(x: jax.Array):
    dma = pltpu.SemaphoreType.DMA
    return pl.pallas_call(
        _kernel,
        out_shape=jax.ShapeDtypeStruct((M, N), jnp.bfloat16),
        in_specs=[pl.BlockSpec(memory_space=pltpu.HBM)],
        out_specs=pl.BlockSpec(memory_space=pltpu.VMEM),
        scratch_shapes=[
            pltpu.VMEM((M, N), jnp.float32),
            *(pltpu.VMEM((8 * (RAW + 2 * RAW_PAIRS), 128), jnp.int32) for _ in range(3)),
            *(pltpu.VMEM((2, HALF, 128), jnp.int32) for _ in range(2)),
            dma((len(LOADS) + 1,)),
            dma,
            dma,
            dma((END,)),
            dma((len(GROUP_ENDS),)),
            dma((3 + RAW_PAIRS,)),
            pltpu.SemaphoreType.REGULAR,
        ],
        compiler_params=pltpu.CompilerParams(
            collective_id=0, disable_bounds_checks=True, disable_semaphore_checks=True
        ),
    )(x)
```

```python
import jax
import jax.numpy as jnp
import numpy as np
from jax import lax
from jax.experimental import pallas as pl
from jax.experimental.pallas import tpu as pltpu

M, N = 1024, 512
HALF = M // 2
UNITS = HALF // 8

WORDS = 17
FULL = 14
POOL = 7
STACK = 1
SIGNS = STACK + FULL
LOW = SIGNS + UNITS // 8
END = LOW + UNITS
EXTRA = 10
SPLIT = END - EXTRA
RAW = END + EXTRA
RAW_PAIRS = (UNITS - FULL) // 2

EARLY = 24
LATE = LOW + EARLY
SEND_ORDER = (*range(LOW, LATE), *range(SIGNS, LOW), *range(SIGNS), *range(LATE, END))
LOADS = (1, 1, 2) + (4,) * 15
GREET = 32
FIRST_FORWARD = 56
LEAD = 28
OTHER_AT = 66
DECODES = 4
GROUP_ENDS = (LATE, 59, 67, 71, 74, 76, SPLIT, SPLIT + 4, SPLIT + 7, SPLIT + 9, END)
GROUPS = [(start, stop - start) for start, stop in zip((0,) + GROUP_ENDS, GROUP_ENDS)]


def _i32(bits):
    return np.uint32(bits).astype(np.int32)


def _bytes(b):
    return _i32(b * 0x01010101)


EVEN, ODD = _i32(0x00FF00FF), _i32(0xFF00FF00)
SIGN, BORROW = _i32(0x80008000), _i32(0x01000100)


def _shl(a, n):
    return lax.shift_left(a, np.int32(n) if isinstance(n, int) else n)


def _shr(a, n):
    return lax.shift_right_logical(a, np.int32(n) if isinstance(n, int) else n)


def _rows(unit, count=1):
    start = 8 * unit
    return pl.ds(start if isinstance(start, int) else pl.multiple_of(start, 8), 8 * count)


def _live(j):
    n = 4 * (j + 1)
    return min(j + 1, WORDS, int(np.ceil((1.68 * n + 5.8 * np.sqrt(n) + 10) / 32)))


def _to_pairs(rows):
    tiles = [rows[:, c : c + 128].reshape(-1, 8, 128) for c in range(0, N, 128)]
    pairs = (jnp.concatenate(tiles[i : i + 2], axis=1).reshape(-1, 128) for i in (0, 2))
    return tuple(pltpu.bitcast(p.astype(jnp.bfloat16), jnp.int32) for p in pairs)


def _from_pairs(u, v):
    pairs = (pltpu.bitcast(w, jnp.bfloat16).astype(jnp.float32) for w in (u, v))
    tiles = [p.reshape(-1, 16, 128)[:, r : r + 8] for p in pairs for r in (0, 8)]
    return jnp.concatenate([t.reshape(-1, 128) for t in tiles], axis=1)


def _low_bytes(u, v):
    return (u & EVEN) | _shl(v & EVEN, 8)


def _high_bytes(u, v):
    return (_shr(u, 8) & EVEN) | (v & ODD)


def _reference(pairs):
    total = sum((w & 0x7FFF) + (_shr(w, 16) & 0x7FFF) for w in pairs).astype(jnp.float32)
    total = jnp.sum(jnp.sum(total, axis=1, keepdims=True), axis=0, keepdims=True)
    mean = jnp.broadcast_to(total, (8, 128)) * (1.0 / (2 * sum(w.size for w in pairs)))
    return jnp.minimum(mean.astype(jnp.int32) + 516, 0x7FFF)


def _sublane():
    return lax.broadcasted_iota(jnp.int32, (8, 128), 0)


def _or_sublanes(a):
    for shift in (4, 2, 1):
        a = a | pltpu.roll(a, shift, 0)
    return a


def _pooled(counts, sublanes):
    counts &= _shl(jnp.ones_like(counts), 2 * sublanes) - 1
    return lax.population_count(counts) + lax.population_count(counts & 0xAAAA)


class _Encoder:
    def __init__(self, k):
        self.k = k
        self.k2 = k | _shl(k, 16) | SIGN
        zero = jnp.zeros_like(k)
        self.words = None
        self.bits, self.room, self.long, self.below_k = zero, zero, zero, ~zero

    def push(self, first, u, v):
        d = _high_bytes(*(self.k2[None] - (w.reshape(-1, 8, 128) & ~SIGN) for w in (u, v)))
        ge1, ge4 = (d - _bytes(1)) & _bytes(0x80), (d - _bytes(4)) & _bytes(0x80)
        size = (d - _bytes(0x7C)) + _shr(ge4, 7) - _shr(ge1, 5)
        end = size + _shl(size, 8)
        end = end + _shl(end, 16)
        one = jnp.ones_like(end)
        code = (one | _shl(one, end & 31)) | (
            _shl(one, _shr(end, 8) & 31) | _shl(one, _shr(end, 16) & 31)
        )
        long, bits = size | end, _shr(end, 24)
        for i, j in enumerate(range(first, first + d.shape[0])):
            self.below_k &= d[i]
            self.long |= long[i]
            self.bits += bits[i]
            if j == UNITS - 1 or _live(j + 1) != _live(j):
                self.room |= 32 * _live(j) - self.bits
            n, new = bits[i : i + 1] & 31, code[i : i + 1]
            if j == 0:
                self.words = _shl(new, -n & 31)
                continue
            old, kept = self.words, _shr(self.words, n)
            if _live(j) > old.shape[0]:
                kept = jnp.concatenate([kept, jnp.zeros_like(new)])
            self.words = kept | _shl(jnp.concatenate([new, old])[: _live(j)], -n & 31)

    def header(self):
        misfit = (self.long & _bytes(0xE0)) | (~self.below_k & _bytes(0x80))
        misfit = jnp.where((misfit != 0) | (self.room < 0), 1, 0)
        fills = [self.bits > 32 * i for i in range(FULL, WORDS)]
        counts = _or_sublanes(_shl(sum(jnp.where(f, 1, 0) for f in fills), 2 * _sublane()))
        misfit = _or_sublanes(misfit) | jnp.where(_pooled(counts, 8) > POOL, 1, 0)
        head = self.k | _shl(misfit, 15) | _shl(counts, 16)
        place = _pooled(counts, _sublane())
        for row in range(POOL):
            word = sum(
                jnp.where(f & (place == row - i), self.words[FULL + i], 0)
                for i, f in enumerate(fills)
            )
            head = jnp.where(_sublane() == 1 + row, _or_sublanes(word), head)
        return head


class _Decoder:
    def __init__(self, wire, uncoded):
        self.wire = wire

        def row(i):
            return jnp.broadcast_to(wire[pl.ds(i, 1), :], (8, 128))

        head = row(0)
        place = _pooled(_shr(head, 16), _sublane())
        pooled = [head] * (WORDS - FULL)
        for j in range(POOL):
            word = row(1 + j)
            pooled = [jnp.where(place == j - i, word, w) for i, w in enumerate(pooled)]
        words = jnp.concatenate([wire[_rows(STACK, FULL), :]] + pooled).reshape(WORDS, 8, 128)
        self.words = jnp.where(uncoded, -1, words)
        k = jnp.where(uncoded, 0xFF, head & 0x7FFF)
        high, low = _shl(_shr(k, 8) - 1, 8), (k & 0xFF) | 0x100
        self.k_high, self.k_low = high + _shl(high, 16), low | _shl(low, 16)
        self.left = UNITS
        self._scan()

    def _scan(self):
        word = self.words[0]
        self.zeros = [lax.clz(word)]
        for _ in range(3):
            word = _shl(_shl(word, 1), self.zeros[-1])
            self.zeros.append(lax.clz(word))

    def pop(self, count):
        popped = []
        for _ in range(count):
            j = self.left = self.left - 1
            signs = _shl(self.wire[_rows(SIGNS + j // 8), :], 2 * (j % 8))
            popped.insert(0, (*self.zeros, signs))
            if j:
                n = (self.zeros[0] + 4) + self.zeros[1] + self.zeros[2]
                n, rest = (n + self.zeros[3])[None], ((32 - n) - self.zeros[3])[None]
                old, live = self.words, _live(j - 1)
                below = _shr(old[1 : live + 1], rest)
                if below.shape[0] < live:
                    below = jnp.concatenate([below, jnp.zeros_like(n)])
                self.words = _shl(old[:live], n) | below
                self._scan()
        z3, z2, z1, z0, signs = (jnp.concatenate(a) for a in zip(*popped))
        rank = (z0 | _shl(z1, 8)) | (_shl(z2, 16) | _shl(z3, 24))
        ge3, ge4 = (rank + _bytes(0x7D)) & _bytes(0x80), (rank + _bytes(0x7C)) & _bytes(0x80)
        d = (rank + _bytes(1)) - _shr(ge3 ^ ge4, 5) - _shr(ge4, 7)
        k_high = jnp.concatenate([self.k_high] * count)
        return (
            k_high - _shl(d & EVEN, 8) + (signs & SIGN),
            k_high - (d & ODD) + (_shl(signs, 1) & SIGN),
        )

    def join(self, low, hu, hv):
        k_low = jnp.concatenate([self.k_low] * (low.shape[0] // 8))
        lu, lv = low & EVEN, _shr(low, 8) & EVEN
        return hu + lu + ((k_low - lu) & BORROW), hv + lv + ((k_low - lv) & BORROW)


def _kernel(
    x_hbm, out_ref, x_ref, tx, from_y, from_x, high_y, high_x,
    load_sems, y_sent, x_sent, y_sems, x_sems, raw_sems, x_started,
):
    my_x, my_y = lax.axis_index("x"), lax.axis_index("y")
    y_peer, x_peer = (my_x, 1 - my_y), (1 - my_x, my_y)
    mine, other = my_x * UNITS, (1 - my_x) * UNITS

    def remote(src, dst, send_sem, recv_sem, peer):
        return pltpu.make_async_remote_copy(
            src, dst, send_sem, recv_sem, device_id=peer, device_id_type=pl.DeviceIdType.MESH
        )

    def signal(sem, peer):
        pl.semaphore_signal(sem, inc=1, device_id=peer, device_id_type=pl.DeviceIdType.MESH)

    def y_copy(p):
        part = _rows(SEND_ORDER[p])
        return remote(tx.at[part], from_y.at[part], y_sent, y_sems.at[p], y_peer)

    def x_copy(p):
        part = _rows(SEND_ORDER[p])
        group = sum(p >= end for end in GROUP_ENDS)
        return remote(from_y.at[part], from_x.at[part], x_sent, x_sems.at[group], x_peer)

    def raw_y_copy(i, pairs=1):
        part = _rows(RAW + 2 * i, 2 * pairs)
        return remote(tx.at[part], from_y.at[part], raw_sems.at[0], raw_sems.at[3 + i], y_peer)

    def raw_x_copy(i, pairs=1):
        part = _rows(RAW + 2 * i, 2 * pairs)
        return remote(from_y.at[part], from_x.at[part], raw_sems.at[1], raw_sems.at[2], x_peer)

    def raw_rows(j):
        return _rows(jnp.where(j < FULL, STACK + j, RAW + j - FULL))

    def misfits(wire):
        bit = wire[pl.ds(0, 1), :] & 0x8000
        return jnp.max(bit.astype(jnp.float32), axis=1, keepdims=True)

    barrier = pltpu.get_barrier_semaphore()
    loads, first = {}, 0
    for i, n in enumerate(LOADS):
        loads[first] = pltpu.make_async_copy(
            x_hbm.at[_rows(mine + first, n)], x_ref.at[_rows(first, n)], load_sems.at[i]
        )
        loads[first].start()
        first += n
        if i == 0:
            signal(barrier, y_peer)
            pl.when(my_x == 0)(lambda: signal(barrier, x_peer))
    load_other = pltpu.make_async_copy(
        x_hbm.at[_rows(other, UNITS)], x_ref.at[_rows(UNITS, UNITS)], load_sems.at[len(LOADS)]
    )
    load_other.start()

    def greet():
        pl.semaphore_wait(barrier, 1 + my_x)
        y_copy(0).start()
        pl.when(my_x == 1)(lambda: signal(x_started, x_peer))

    def forward(p):
        y_copy(p).wait_recv()
        if p == 0:
            pl.when(my_x == 0)(lambda: pl.semaphore_wait(x_started, 1))
        if p < SPLIT:
            x_copy(p).start()
        else:
            pl.when(my_x == 0)(lambda: x_copy(p).start())

    sent = arrived = 0
    todo = []
    for j, n in zip(loads, LOADS):
        loads[j].wait()
        u, v = _to_pairs(x_ref[_rows(j, n), :])
        tx[_rows(LOW + j, n), :] = _low_bytes(u, v)
        if j < EARLY:

            @pl.when(my_y == 1)
            def _():
                for p in range(j, j + n):
                    y_copy(p).start() if p else greet()

            sent += n
        if j + n == GREET:

            @pl.when(my_y == 0)
            def _():
                greet()
                for p in range(1, sent):
                    y_copy(p).start()

        todo.append((j, u, v))
        if j == 1:
            encoder = _Encoder(_reference([w for _, *pair in todo for w in pair]))
        while j >= 1 and todo:
            encoder.push(*todo.pop(0))
        for i in range(n):
            pair = (u[8 * i : 8 * i + 8] & SIGN) | _shr(v[8 * i : 8 * i + 8] & SIGN, 1)
            signs = signs | _shr(pair, 2 * ((j + i) % 8)) if (j + i) % 8 else pair
        if (j + n) % 8 == 0:
            tx[_rows(SIGNS + j // 8), :] = signs
        while j >= GREET and sent < EARLY + (j + n) // 8:
            y_copy(sent).start()
            sent += 1
        if j + n >= FIRST_FORWARD:
            forward(arrived)
            arrived += 1
    tx[_rows(STACK, FULL), :] = encoder.words[:FULL].reshape(-1, 128)
    forward(arrived)
    tx[_rows(0), :] = encoder.header()
    forward(arrived + 1)
    found = misfits(tx)
    forward(arrived + 2)
    mine_uncoded = found[0, 0] > 0
    forward(arrived + 3)

    @pl.when(mine_uncoded)
    def _():
        @pl.loop(0, UNITS)
        def _(j):
            tx[raw_rows(j), :] = _high_bytes(*_to_pairs(x_ref[_rows(j), :]))

    def wait_group(i):
        part = from_x.at[_rows(*GROUPS[i])]
        pltpu.make_async_copy(part, part, x_sems.at[i]).wait()

    decoders = []

    def decode(count):
        for decoder, high in zip(decoders, (high_y, high_x)):
            while n := min(decoder.left, count, DECODES):
                count -= n
                eu, ev = decoder.pop(n)
                high[0, _rows(decoder.left, n), :], high[1, _rows(decoder.left, n), :] = eu, ev

    for p in range(arrived + 4, END):
        forward(p)
        for _ in range(3):
            if sent < min(END, p + LEAD):
                y_copy(sent).start()
                sent += 1
        if sent == END:
            sent += EXTRA

            @pl.when(my_x == 0)
            def _():
                for i, (start, n) in enumerate(GROUPS):
                    if start >= SPLIT:
                        src, dst = tx.at[_rows(start + EXTRA, n)], from_x.at[_rows(start, n)]
                        remote(src, dst, y_sent, x_sems.at[i], y_peer).start()

            @pl.when(mine_uncoded)
            def _():
                pl.loop(0, RAW_PAIRS)(lambda i: raw_y_copy(i).start())

        if p == EARLY:
            load_other.wait()

            @pl.when(my_x == 0)
            def _():
                pairs = _to_pairs(x_ref[_rows(2 * UNITS - EXTRA, EXTRA), :])
                tx[_rows(END, EXTRA), :] = _low_bytes(*pairs)

        elif p == SEND_ORDER.index(0):
            found = misfits(from_y)
        elif p == SEND_ORDER.index(0) + 1:
            y_uncoded = found[0, 0] > 0
        elif p == LATE - 1:
            decoders.append(_Decoder(from_y, y_uncoded))
        elif p == OTHER_AT:
            wait_group(0)
            found = misfits(from_x)
        elif p == OTHER_AT + 1:
            x_uncoded = found[0, 0] > 0
        elif p == OTHER_AT + 2:
            decoders.append(_Decoder(from_x, x_uncoded))
        else:
            decode(DECODES)
    assert sent == END + EXTRA
    decode(2 * UNITS)

    def use_raw(wire, high):
        @pl.loop(0, UNITS)
        def _(j):
            raw = wire[raw_rows(j), :]
            high[0, _rows(j), :] = _shl(raw & EVEN, 8) - BORROW
            high[1, _rows(j), :] = (raw & ODD) - BORROW

    @pl.when(mine_uncoded | y_uncoded | x_uncoded)
    def _():
        @pl.when(y_uncoded)
        def _():
            @pl.loop(0, RAW_PAIRS)
            def _(i):
                raw_y_copy(i).wait_recv()
                raw_x_copy(i).start()

            use_raw(from_y, high_y)
            raw_x_copy(0, RAW_PAIRS).wait_send()

        @pl.when(x_uncoded)
        def _():
            raw_x_copy(0, RAW_PAIRS).wait_recv()
            use_raw(from_x, high_x)

        pl.when(mine_uncoded)(lambda: raw_y_copy(0, RAW_PAIRS).wait_send())

    def add(half, start, stop):
        wire, high, first = ((from_y, high_y, mine), (from_x, high_x, other))[half]
        for j in range(start, stop, 4):
            n = min(4, stop - j)
            pairs = decoders[half].join(
                wire[_rows(LOW + j, n), :], high[0, _rows(j, n), :], high[1, _rows(j, n), :]
            )
            total = x_ref[_rows(half * UNITS + j, n), :] + _from_pairs(*pairs)
            out_ref[_rows(first + j, n), :] = total.astype(out_ref.dtype)

    def wait_sent(y_units, x_units):
        y_part, x_part = _rows(0, y_units), _rows(0, x_units)
        remote(tx.at[y_part], from_y.at[y_part], y_sent, y_sems.at[0], y_peer).wait_send()
        remote(from_y.at[x_part], from_x.at[x_part], x_sent, x_sems.at[0], x_peer).wait_send()

    add(0, 0, UNITS)
    add(1, 0, EARLY)
    order = sorted(
        range(1, len(GROUP_ENDS)), key=lambda i: GROUP_ENDS[i] - EXTRA * (GROUP_ENDS[i] > SPLIT)
    )
    for i in order:
        if i == order[-2]:
            pl.when(my_x == 0)(lambda: wait_sent(END + EXTRA, END))
            pl.when(my_x == 1)(lambda: wait_sent(END, SPLIT))
        wait_group(i)
        add(1, GROUP_ENDS[i - 1] - LOW, GROUP_ENDS[i] - LOW)


def pallas_dist_ar_xy_y_m1024_n512_kernel(x: jax.Array):
    dma = pltpu.SemaphoreType.DMA
    return pl.pallas_call(
        _kernel,
        out_shape=jax.ShapeDtypeStruct((M, N), jnp.bfloat16),
        in_specs=[pl.BlockSpec(memory_space=pltpu.HBM)],
        out_specs=pl.BlockSpec(memory_space=pltpu.VMEM),
        scratch_shapes=[
            pltpu.VMEM((M, N), jnp.float32),
            *(pltpu.VMEM((8 * (RAW + 2 * RAW_PAIRS), 128), jnp.int32) for _ in range(3)),
            *(pltpu.VMEM((2, HALF, 128), jnp.int32) for _ in range(2)),
            dma((len(LOADS) + 1,)),
            dma,
            dma,
            dma((END,)),
            dma((len(GROUP_ENDS),)),
            dma((3 + RAW_PAIRS,)),
            pltpu.SemaphoreType.REGULAR,
        ],
        compiler_params=pltpu.CompilerParams(
            collective_id=0, disable_bounds_checks=True, disable_semaphore_checks=True
        ),
    )(x)
```
